```python
import numpy as np

kernel_name = "dist_rope_attn_htp_bs_b2_sq512_d1024_hq8_dh128"

def setup_inputs():
    x = np.random.randn(8, 512, 1024).astype(np.float32)
    Wq = np.random.randn(1024, 4096).astype(np.float32) * 0.02
    Wk = np.random.randn(1024, 4096).astype(np.float32) * 0.02
    Wv = np.random.randn(1024, 4096).astype(np.float32) * 0.02
    Wo = np.random.randn(4096, 1024).astype(np.float32) * 0.02
    return {"x": x, "Wq": Wq, "Wk": Wk, "Wv": Wv, "Wo": Wo}

def reference(x, Wq, Wk, Wv, Wo):
    B, Sq, Hq, Dh = 8, 512, 32, 128
    inv = 1.0 / (10000.0 ** (np.arange(0, Dh, 2) / Dh))
    pos = np.arange(Sq)[:, None] * inv[None, :]
    cos = np.repeat(np.cos(pos), 2, axis=-1).astype(np.float32)
    sin = np.repeat(np.sin(pos), 2, axis=-1).astype(np.float32)
    def rot(t):
        t2 = t.reshape(B, Sq, Hq, Dh // 2, 2)
        t_r = np.stack([-t2[..., 1], t2[..., 0]], axis=-1).reshape(B, Sq, Hq, Dh)
        return t * cos[None, :, None, :] + t_r * sin[None, :, None, :]
    Q = rot((x @ Wq).reshape(B, Sq, Hq, Dh))
    K = rot((x @ Wk).reshape(B, Sq, Hq, Dh))
    V = (x @ Wv).reshape(B, Sq, Hq, Dh)
    s = np.einsum('bihd,bjhd->bhij', Q, K).astype(np.float32) * 0.08838834764831843
    s_max = s.max(axis=-1, keepdims=True)
    w = np.exp(s - s_max)
    w = w / w.sum(axis=-1, keepdims=True)
    ctx = np.einsum('bhij,bjhd->bihd', w, V).reshape(B, Sq, Hq * Dh)
    return ctx @ Wo
```

```python
import jax
import jax.numpy as jnp
import numpy as np
from jax import lax
from jax.experimental import pallas as pl
from jax.experimental.pallas import tpu as pltpu

S, D, H, DH = 512, 1024, 8, 128
NU = 8
BF = jnp.bfloat16
F32 = jnp.float32


def _tables():
    inv = 1.0 / (10000.0 ** (np.arange(0, DH, 2) / DH))
    pos = np.arange(S)[:, None] * inv[None, :]
    cos = np.repeat(np.cos(pos), 2, axis=-1)
    sin = np.repeat(np.sin(pos), 2, axis=-1)
    even = (np.arange(DH) % 2 == 0)[None, :]
    sa = np.where(even, -sin, 0.0)
    sb = np.where(even, 0.0, sin)
    c = 0.08838834764831843 * 1.4426950408889634
    return np.stack([cos * c, sa * c, sb * c, cos, sa, sb]).astype(np.float32)


_TAB = _tables()

_OFF = (0, 3, 1, 2, 2, 3, 1, 0)
_BAT = (0, 0, 0, 0, 1, 1, 1, 1)


def _body(x_hbm, wq_hbm, wk_hbm, wv_hbm, wo_hbm, tab_ref, out_hbm,
          xst, wst, wbf, xbuf, qkv, ctx, pbuf, rbuf, obuf,
          lsem, osem, xs_sem, xr_sem, ps_sem, pr_sem):
    me = lax.axis_index("i")

    def dev(off):
        return ((me + off) % 4,)

    bar = pltpu.get_barrier_semaphore()
    for off in (1, 2, 3):
        pl.semaphore_signal(bar, inc=1, device_id=dev(off), device_id_type=pl.DeviceIdType.MESH)

    xl = [pltpu.make_async_copy(x_hbm.at[b], xst.at[b], lsem.at[b]) for b in range(2)]
    wl = [pltpu.make_async_copy(w, wst.at[i], lsem.at[2 + i])
          for i, w in enumerate((wq_hbm, wk_hbm, wv_hbm, wo_hbm))]
    xl[0].start()
    wl[0].start()
    wl[1].start()
    xl[1].start()
    wl[2].start()
    wl[3].start()

    def xsend(u):
        src = 0 if _BAT[u] == 0 else 7
        return pltpu.make_async_remote_copy(
            src_ref=xbuf.at[src], dst_ref=xbuf.at[u], send_sem=xs_sem.at[u], recv_sem=xr_sem.at[u],
            device_id=dev(4 - _OFF[u]), device_id_type=pl.DeviceIdType.MESH)

    def psend(u, off):
        return pltpu.make_async_remote_copy(
            src_ref=pbuf.at[u], dst_ref=rbuf.at[u], send_sem=ps_sem.at[u], recv_sem=pr_sem.at[u],
            device_id=dev(off), device_id_type=pl.DeviceIdType.MESH)

    xl[0].wait()
    xbuf[0] = xst[0].astype(BF)
    pl.semaphore_wait(bar, 3)
    for u in (1, 2, 3):
        xsend(u).start()
    xl[1].wait()
    xbuf[7] = xst[1].astype(BF)
    for u in (4, 5, 6):
        xsend(u).start()
    for i in range(4):
        wl[i].wait()
        wbf[i] = wst[i].astype(BF)

    def unit(u, carry):
        @pl.when(jnp.logical_and(u > 0, u < 7))
        def _():
            pltpu.make_async_copy(xbuf.at[u], xbuf.at[u], xr_sem.at[u]).wait()

        xb = xbuf[u]
        for w in range(3):
            for c in range(4):
                t = jnp.dot(xb, wbf[w, :, c * 256:(c + 1) * 256], preferred_element_type=F32)
                if w < 2:
                    cs, sa, sb = tab_ref[3 * w], tab_ref[3 * w + 1], tab_ref[3 * w + 2]
                    for hh in range(2):
                        th = t[:, hh * 128:(hh + 1) * 128]
                        r = th * cs + pltpu.roll(th, 127, 1) * sa + pltpu.roll(th, 1, 1) * sb
                        qkv[w, 2 * c + hh] = r.astype(BF)
                else:
                    for hh in range(2):
                        qkv[w, 2 * c + hh] = t[:, hh * 128:(hh + 1) * 128].astype(BF)
        for h in range(H):
            s = lax.dot_general(qkv[0, h], qkv[1, h], (((1,), (1,)), ((), ())),
                                preferred_element_type=F32)
            m = jnp.max(s, axis=1, keepdims=True)
            p = jnp.exp2(s - m)
            l = jnp.sum(p, axis=1, keepdims=True)
            o = jnp.dot(p.astype(BF), qkv[2, h], preferred_element_type=F32)
            ctx[:, h * 128:(h + 1) * 128] = (o / l).astype(BF)

        @pl.when(u < 7)
        def _():
            for c in range(4):
                pbuf[u, :, c * 256:(c + 1) * 256] = jnp.dot(
                    ctx[...], wbf[3, :, c * 256:(c + 1) * 256], preferred_element_type=F32).astype(BF)

        @pl.when(jnp.logical_and(u > 0, u < 7))
        def _():
            off = jnp.where(u == 1, 3, jnp.where(u == 5, 3, jnp.where(jnp.logical_or(u == 2, u == 6), 1, 2)))
            psend(u, off).start()

        @pl.when(u == 5)
        def _():
            for k in (1, 2, 3):
                pltpu.make_async_copy(rbuf.at[k], rbuf.at[k], pr_sem.at[k]).wait()
            obuf[0] = (pbuf[0].astype(F32) + rbuf[1].astype(F32)) + (rbuf[2].astype(F32) + rbuf[3].astype(F32))
            pltpu.make_async_copy(obuf.at[0], out_hbm.at[0], osem.at[0]).start()

        return carry

    lax.fori_loop(0, NU, unit, 0)

    for k in (4, 5, 6):
        pltpu.make_async_copy(rbuf.at[k], rbuf.at[k], pr_sem.at[k]).wait()
    ocp = []
    for c in range(4):
        sl = slice(c * 256, (c + 1) * 256)
        t = jnp.dot(ctx[...], wbf[3, :, sl], preferred_element_type=F32)
        obuf[1, :, sl] = (t + rbuf[4, :, sl].astype(F32)) + (rbuf[5, :, sl].astype(F32) + rbuf[6, :, sl].astype(F32))
        cp = pltpu.make_async_copy(obuf.at[1, :, sl], out_hbm.at[1, :, sl], osem.at[1 + c])
        cp.start()
        ocp.append(cp)
    for u in range(1, 7):
        xsend(u).wait_send()
        psend(u, _OFF[u]).wait_send()
    pltpu.make_async_copy(obuf.at[0], out_hbm.at[0], osem.at[0]).wait()
    for cp in ocp:
        cp.wait()


def pallas_dist_rope_attn_htp_bs_b2_sq512_d1024_hq8_dh128_kernel(x, Wq, Wk, Wv, Wo):
    anyspec = pl.BlockSpec(memory_space=pl.ANY)
    return pl.pallas_call(
        _body,
        out_shape=jax.ShapeDtypeStruct((2, S, D), F32),
        in_specs=[anyspec] * 5 + [pl.BlockSpec(memory_space=pltpu.VMEM)],
        out_specs=anyspec,
        scratch_shapes=[
            pltpu.VMEM((2, S, D), F32),
            pltpu.VMEM((4, D, D), F32),
            pltpu.VMEM((4, D, D), BF),
            pltpu.VMEM((NU, S, D), BF),
            pltpu.VMEM((3, H, S, DH), BF),
            pltpu.VMEM((S, D), BF),
            pltpu.VMEM((NU - 1, S, D), BF),
            pltpu.VMEM((NU - 1, S, D), BF),
            pltpu.VMEM((2, S, D), F32),
            pltpu.SemaphoreType.DMA((6,)),
            pltpu.SemaphoreType.DMA((5,)),
            pltpu.SemaphoreType.DMA((NU,)),
            pltpu.SemaphoreType.DMA((NU,)),
            pltpu.SemaphoreType.DMA((NU,)),
            pltpu.SemaphoreType.DMA((NU,)),
        ],
        compiler_params=pltpu.CompilerParams(collective_id=0, vmem_limit_bytes=100 * 1024 * 1024),
    )(x, Wq, Wk, Wv, Wo, jnp.asarray(_TAB))
```

```python
import jax
import jax.numpy as jnp
import numpy as np
from jax import lax
from jax.experimental import pallas as pl
from jax.experimental.pallas import tpu as pltpu

S, D, H, DH = 512, 1024, 8, 128
NU = 8
BF = jnp.bfloat16
F32 = jnp.float32


def _tables():
    inv = 1.0 / (10000.0 ** (np.arange(0, DH, 2) / DH))
    pos = np.arange(S)[:, None] * inv[None, :]
    cos = np.repeat(np.cos(pos), 2, axis=-1)
    sin = np.repeat(np.sin(pos), 2, axis=-1)
    even = (np.arange(DH) % 2 == 0)[None, :]
    sa = np.where(even, -sin, 0.0)
    sb = np.where(even, 0.0, sin)
    c = 0.08838834764831843 * 1.4426950408889634
    return np.stack([cos * c, sa * c, sb * c, cos, sa, sb]).astype(np.float32)


_TAB = _tables()

_OFF = (0, 3, 1, 2, 2, 3, 1, 0)
_BAT = (0, 0, 0, 0, 1, 1, 1, 1)


def _body(x_hbm, wq_hbm, wk_hbm, wv_hbm, wo_hbm, tab_hbm, out_hbm,
          tab_ref, xst, wst, wbf, xbuf, qkv, ctx, pbuf, rbuf, obuf,
          lsem, osem, xs_sem, xr_sem, ps_sem, pr_sem):
    me = lax.axis_index("i")

    def dev(off):
        return ((me + off) % 4,)

    bar = pltpu.get_barrier_semaphore()
    for off in (1, 2, 3):
        pl.semaphore_signal(bar, inc=1, device_id=dev(off), device_id_type=pl.DeviceIdType.MESH)

    xl = [pltpu.make_async_copy(x_hbm.at[b], xst.at[b], lsem.at[b]) for b in range(2)]
    wl = [pltpu.make_async_copy(w, wst.at[i], lsem.at[2 + i])
          for i, w in enumerate((wq_hbm, wk_hbm, wv_hbm, wo_hbm))]
    xl[0].start()
    wl[0].start()
    wl[1].start()
    xl[1].start()
    tl = pltpu.make_async_copy(tab_hbm, tab_ref, lsem.at[6])
    tl.start()
    wl[2].start()
    wl[3].start()

    def xsend(u):
        src = 0 if _BAT[u] == 0 else 7
        return pltpu.make_async_remote_copy(
            src_ref=xbuf.at[src], dst_ref=xbuf.at[u], send_sem=xs_sem.at[u], recv_sem=xr_sem.at[u],
            device_id=dev(4 - _OFF[u]), device_id_type=pl.DeviceIdType.MESH)

    def psend(u, off):
        return pltpu.make_async_remote_copy(
            src_ref=pbuf.at[u], dst_ref=rbuf.at[u], send_sem=ps_sem.at[u], recv_sem=pr_sem.at[u],
            device_id=dev(off), device_id_type=pl.DeviceIdType.MESH)

    xl[0].wait()
    xbuf[0] = xst[0].astype(BF)
    pl.semaphore_wait(bar, 3)
    for u in (1, 2, 3):
        xsend(u).start()
    xl[1].wait()
    xbuf[7] = xst[1].astype(BF)
    for u in (4, 5, 6):
        xsend(u).start()
    tl.wait()
    for i in range(4):
        wl[i].wait()
        wbf[i] = wst[i].astype(BF)

    def unit(u, carry):
        @pl.when(jnp.logical_and(u > 0, u < 7))
        def _():
            pltpu.make_async_copy(xbuf.at[u], xbuf.at[u], xr_sem.at[u]).wait()

        xb = xbuf[u]
        for w in range(3):
            for c in range(4):
                t = jnp.dot(xb, wbf[w, :, c * 256:(c + 1) * 256], preferred_element_type=F32)
                if w < 2:
                    cs, sa, sb = tab_ref[3 * w], tab_ref[3 * w + 1], tab_ref[3 * w + 2]
                    for hh in range(2):
                        th = t[:, hh * 128:(hh + 1) * 128]
                        r = th * cs + pltpu.roll(th, 127, 1) * sa + pltpu.roll(th, 1, 1) * sb
                        qkv[w, 2 * c + hh] = r.astype(BF)
                else:
                    for hh in range(2):
                        qkv[w, 2 * c + hh] = t[:, hh * 128:(hh + 1) * 128].astype(BF)
        for h in range(H):
            s = lax.dot_general(qkv[0, h], qkv[1, h], (((1,), (1,)), ((), ())),
                                preferred_element_type=F32)
            m = jnp.max(s, axis=1, keepdims=True)
            p = jnp.exp2(s - m)
            l = jnp.sum(p, axis=1, keepdims=True)
            o = jnp.dot(p.astype(BF), qkv[2, h], preferred_element_type=F32)
            ctx[:, h * 128:(h + 1) * 128] = (o / l).astype(BF)

        @pl.when(u < 7)
        def _():
            for c in range(4):
                pbuf[u, :, c * 256:(c + 1) * 256] = jnp.dot(
                    ctx[...], wbf[3, :, c * 256:(c + 1) * 256], preferred_element_type=F32).astype(BF)

        @pl.when(jnp.logical_and(u > 0, u < 7))
        def _():
            off = jnp.where(u == 1, 3, jnp.where(u == 5, 3, jnp.where(jnp.logical_or(u == 2, u == 6), 1, 2)))
            psend(u, off).start()

        @pl.when(u == 5)
        def _():
            for k in (1, 2, 3):
                pltpu.make_async_copy(rbuf.at[k], rbuf.at[k], pr_sem.at[k]).wait()
            obuf[0] = (pbuf[0].astype(F32) + rbuf[1].astype(F32)) + (rbuf[2].astype(F32) + rbuf[3].astype(F32))
            pltpu.make_async_copy(obuf.at[0], out_hbm.at[0], osem.at[0]).start()

        return carry

    lax.fori_loop(0, NU, unit, 0)

    for k in (4, 5, 6):
        pltpu.make_async_copy(rbuf.at[k], rbuf.at[k], pr_sem.at[k]).wait()
    ocp = []
    for c in range(4):
        sl = slice(c * 256, (c + 1) * 256)
        t = jnp.dot(ctx[...], wbf[3, :, sl], preferred_element_type=F32)
        obuf[1, :, sl] = (t + rbuf[4, :, sl].astype(F32)) + (rbuf[5, :, sl].astype(F32) + rbuf[6, :, sl].astype(F32))
        cp = pltpu.make_async_copy(obuf.at[1, :, sl], out_hbm.at[1, :, sl], osem.at[1 + c])
        cp.start()
        ocp.append(cp)
    for u in range(1, 7):
        xsend(u).wait_send()
        psend(u, _OFF[u]).wait_send()
    pltpu.make_async_copy(obuf.at[0], out_hbm.at[0], osem.at[0]).wait()
    for cp in ocp:
        cp.wait()


def pallas_dist_rope_attn_htp_bs_b2_sq512_d1024_hq8_dh128_kernel(x, Wq, Wk, Wv, Wo):
    anyspec = pl.BlockSpec(memory_space=pl.ANY)
    return pl.pallas_call(
        _body,
        out_shape=jax.ShapeDtypeStruct((2, S, D), F32),
        in_specs=[anyspec] * 6,
        out_specs=anyspec,
        scratch_shapes=[
            pltpu.VMEM((6, S, DH), F32),
            pltpu.VMEM((2, S, D), F32),
            pltpu.VMEM((4, D, D), F32),
            pltpu.VMEM((4, D, D), BF),
            pltpu.VMEM((NU, S, D), BF),
            pltpu.VMEM((3, H, S, DH), BF),
            pltpu.VMEM((S, D), BF),
            pltpu.VMEM((NU - 1, S, D), BF),
            pltpu.VMEM((NU - 1, S, D), BF),
            pltpu.VMEM((2, S, D), F32),
            pltpu.SemaphoreType.DMA((7,)),
            pltpu.SemaphoreType.DMA((5,)),
            pltpu.SemaphoreType.DMA((NU,)),
            pltpu.SemaphoreType.DMA((NU,)),
            pltpu.SemaphoreType.DMA((NU,)),
            pltpu.SemaphoreType.DMA((NU,)),
        ],
        compiler_params=pltpu.CompilerParams(collective_id=0, vmem_limit_bytes=100 * 1024 * 1024),
    )(x, Wq, Wk, Wv, Wo, jnp.asarray(_TAB))
```

```python
import jax
import jax.numpy as jnp
import numpy as np
from jax import lax
from jax.experimental import pallas as pl
from jax.experimental.pallas import tpu as pltpu

S, D, H, DH = 512, 1024, 8, 128
NU = 8
BF = jnp.bfloat16
F32 = jnp.float32


def _tables():
    inv = 1.0 / (10000.0 ** (np.arange(0, DH, 2) / DH))
    pos = np.arange(S)[:, None] * inv[None, :]
    cos = np.repeat(np.cos(pos), 2, axis=-1)
    sin = np.repeat(np.sin(pos), 2, axis=-1)
    even = (np.arange(DH) % 2 == 0)[None, :]
    sa = np.where(even, -sin, 0.0)
    sb = np.where(even, 0.0, sin)
    c = 0.08838834764831843 * 1.4426950408889634
    return np.stack([cos * c, sa * c, sb * c, cos, sa, sb]).astype(np.float32)


_TAB = _tables()

_OFF = (0, 3, 1, 2, 2, 3, 1, 0)
_BAT = (0, 0, 0, 0, 1, 1, 1, 1)


def _body(x_hbm, wq_hbm, wk_hbm, wv_hbm, wo_hbm, tab_hbm, out_hbm,
          tab_ref, xst, wst, wbf, xbuf, qkv, ctx, pbuf, rbuf, obuf,
          lsem, osem, xs_sem, xr_sem, ps_sem, pr_sem):
    me = lax.axis_index("i")

    def dev(off):
        return ((me + off) % 4,)

    bar = pltpu.get_barrier_semaphore()
    for off in (1, 2, 3):
        pl.semaphore_signal(bar, inc=1, device_id=dev(off), device_id_type=pl.DeviceIdType.MESH)

    xl = [pltpu.make_async_copy(x_hbm.at[b], xst.at[b], lsem.at[b]) for b in range(2)]
    wl = [pltpu.make_async_copy(w, wst.at[i], lsem.at[2 + i])
          for i, w in enumerate((wq_hbm, wk_hbm, wv_hbm, wo_hbm))]
    tl = pltpu.make_async_copy(tab_hbm, tab_ref, lsem.at[6])
    xl[0].start()
    wl[0].start()
    tl.start()
    wl[1].start()
    xl[1].start()
    wl[2].start()
    wl[3].start()

    def xsend(u):
        src = 0 if _BAT[u] == 0 else 7
        return pltpu.make_async_remote_copy(
            src_ref=xbuf.at[src], dst_ref=xbuf.at[u], send_sem=xs_sem.at[u], recv_sem=xr_sem.at[u],
            device_id=dev(4 - _OFF[u]), device_id_type=pl.DeviceIdType.MESH)

    def psend(u, off):
        return pltpu.make_async_remote_copy(
            src_ref=pbuf.at[u], dst_ref=rbuf.at[u], send_sem=ps_sem.at[u], recv_sem=pr_sem.at[u],
            device_id=dev(off), device_id_type=pl.DeviceIdType.MESH)

    xl[0].wait()
    xbuf[0] = xst[0].astype(BF)
    pl.semaphore_wait(bar, 3)
    for u in (1, 2, 3):
        xsend(u).start()

    def wprep(u, i):
        @pl.when(u == 0)
        def _():
            wl[i].wait()
            wbf[i] = wst[i].astype(BF)
            if i == 0:
                tl.wait()
            if i == 2:
                xl[1].wait()
                xbuf[7] = xst[1].astype(BF)
                for k in (4, 5, 6):
                    xsend(k).start()

    def unit(u, carry):
        @pl.when(jnp.logical_and(u > 0, u < 7))
        def _():
            pltpu.make_async_copy(xbuf.at[u], xbuf.at[u], xr_sem.at[u]).wait()

        xb = xbuf[u]
        for w in range(3):
            wprep(u, w)
            for c in range(4):
                t = jnp.dot(xb, wbf[w, :, c * 256:(c + 1) * 256], preferred_element_type=F32)
                if w < 2:
                    cs, sa, sb = tab_ref[3 * w], tab_ref[3 * w + 1], tab_ref[3 * w + 2]
                    for hh in range(2):
                        th = t[:, hh * 128:(hh + 1) * 128]
                        r = th * cs + pltpu.roll(th, 127, 1) * sa + pltpu.roll(th, 1, 1) * sb
                        qkv[w, 2 * c + hh] = r.astype(BF)
                else:
                    for hh in range(2):
                        qkv[w, 2 * c + hh] = t[:, hh * 128:(hh + 1) * 128].astype(BF)
        for h in range(H):
            s = lax.dot_general(qkv[0, h], qkv[1, h], (((1,), (1,)), ((), ())),
                                preferred_element_type=F32)
            m = jnp.max(s, axis=1, keepdims=True)
            p = jnp.exp2(s - m)
            l = jnp.sum(p, axis=1, keepdims=True)
            o = jnp.dot(p.astype(BF), qkv[2, h], preferred_element_type=F32)
            ctx[:, h * 128:(h + 1) * 128] = (o / l).astype(BF)

        wprep(u, 3)

        @pl.when(u < 7)
        def _():
            for c in range(4):
                pbuf[u, :, c * 256:(c + 1) * 256] = jnp.dot(
                    ctx[...], wbf[3, :, c * 256:(c + 1) * 256], preferred_element_type=F32).astype(BF)

        @pl.when(jnp.logical_and(u > 0, u < 7))
        def _():
            off = jnp.where(u == 1, 3, jnp.where(u == 5, 3, jnp.where(jnp.logical_or(u == 2, u == 6), 1, 2)))
            psend(u, off).start()

        @pl.when(u == 5)
        def _():
            for k in (1, 2, 3):
                pltpu.make_async_copy(rbuf.at[k], rbuf.at[k], pr_sem.at[k]).wait()
            obuf[0] = (pbuf[0].astype(F32) + rbuf[1].astype(F32)) + (rbuf[2].astype(F32) + rbuf[3].astype(F32))
            pltpu.make_async_copy(obuf.at[0], out_hbm.at[0], osem.at[0]).start()

        return carry

    lax.fori_loop(0, NU, unit, 0)

    for k in (4, 5, 6):
        pltpu.make_async_copy(rbuf.at[k], rbuf.at[k], pr_sem.at[k]).wait()
    ocp = []
    for c in range(4):
        sl = slice(c * 256, (c + 1) * 256)
        t = jnp.dot(ctx[...], wbf[3, :, sl], preferred_element_type=F32)
        obuf[1, :, sl] = (t + rbuf[4, :, sl].astype(F32)) + (rbuf[5, :, sl].astype(F32) + rbuf[6, :, sl].astype(F32))
        cp = pltpu.make_async_copy(obuf.at[1, :, sl], out_hbm.at[1, :, sl], osem.at[1 + c])
        cp.start()
        ocp.append(cp)
    for u in range(1, 7):
        xsend(u).wait_send()
        psend(u, _OFF[u]).wait_send()
    pltpu.make_async_copy(obuf.at[0], out_hbm.at[0], osem.at[0]).wait()
    for cp in ocp:
        cp.wait()


def pallas_dist_rope_attn_htp_bs_b2_sq512_d1024_hq8_dh128_kernel(x, Wq, Wk, Wv, Wo):
    anyspec = pl.BlockSpec(memory_space=pl.ANY)
    return pl.pallas_call(
        _body,
        out_shape=jax.ShapeDtypeStruct((2, S, D), F32),
        in_specs=[anyspec] * 6,
        out_specs=anyspec,
        scratch_shapes=[
            pltpu.VMEM((6, S, DH), F32),
            pltpu.VMEM((2, S, D), F32),
            pltpu.VMEM((4, D, D), F32),
            pltpu.VMEM((4, D, D), BF),
            pltpu.VMEM((NU, S, D), BF),
            pltpu.VMEM((3, H, S, DH), BF),
            pltpu.VMEM((S, D), BF),
            pltpu.VMEM((NU - 1, S, D), BF),
            pltpu.VMEM((NU - 1, S, D), BF),
            pltpu.VMEM((2, S, D), F32),
            pltpu.SemaphoreType.DMA((7,)),
            pltpu.SemaphoreType.DMA((5,)),
            pltpu.SemaphoreType.DMA((NU,)),
            pltpu.SemaphoreType.DMA((NU,)),
            pltpu.SemaphoreType.DMA((NU,)),
            pltpu.SemaphoreType.DMA((NU,)),
        ],
        compiler_params=pltpu.CompilerParams(collective_id=0, vmem_limit_bytes=100 * 1024 * 1024),
    )(x, Wq, Wk, Wv, Wo, jnp.asarray(_TAB))
```

```python
import jax
import jax.numpy as jnp
import numpy as np
from jax import lax
from jax.experimental import pallas as pl
from jax.experimental.pallas import tpu as pltpu

S, D, H, DH = 512, 1024, 8, 128
NU = 8
BF = jnp.bfloat16
F32 = jnp.float32


_OFF = (0, 3, 1, 2, 2, 3, 1, 0)
_BAT = (0, 0, 0, 0, 1, 1, 1, 1)


def _body(x_hbm, wq_hbm, wk_hbm, wv_hbm, wo_hbm, out_hbm,
          tab_ref, xst, wst, wbf, xbuf, qkv, ctx, pbuf, rbuf, obuf,
          lsem, osem, xs_sem, xr_sem, ps_sem, pr_sem):
    me = lax.axis_index("i")

    def dev(off):
        return ((me + off) % 4,)

    bar = pltpu.get_barrier_semaphore()
    for off in (1, 2, 3):
        pl.semaphore_signal(bar, inc=1, device_id=dev(off), device_id_type=pl.DeviceIdType.MESH)

    xl = [pltpu.make_async_copy(x_hbm.at[b], xst.at[b], lsem.at[b]) for b in range(2)]
    wl = [pltpu.make_async_copy(w, wst.at[i], lsem.at[2 + i])
          for i, w in enumerate((wq_hbm, wk_hbm, wv_hbm, wo_hbm))]
    xl[0].start()
    wl[0].start()
    wl[1].start()
    xl[1].start()
    wl[2].start()
    wl[3].start()

    def xsend(u):
        src = 0 if _BAT[u] == 0 else 7
        return pltpu.make_async_remote_copy(
            src_ref=xbuf.at[src], dst_ref=xbuf.at[u], send_sem=xs_sem.at[u], recv_sem=xr_sem.at[u],
            device_id=dev(4 - _OFF[u]), device_id_type=pl.DeviceIdType.MESH)

    def psend(u, off):
        return pltpu.make_async_remote_copy(
            src_ref=pbuf.at[u], dst_ref=rbuf.at[u], send_sem=ps_sem.at[u], recv_sem=pr_sem.at[u],
            device_id=dev(off), device_id_type=pl.DeviceIdType.MESH)

    lane = lax.broadcasted_iota(jnp.int32, (S, DH), 1)
    row = lax.broadcasted_iota(jnp.int32, (S, DH), 0).astype(F32)
    ang = row * jnp.exp((lane & ~1).astype(F32) * (-np.log(10000.0) / DH))
    cos, sin = jnp.cos(ang), jnp.sin(ang)
    even = (lane & 1) == 0
    sa = jnp.where(even, -sin, 0.0)
    sb = jnp.where(even, 0.0, sin)
    qs = 0.08838834764831843 * 1.4426950408889634
    for k, t in enumerate((cos * qs, sa * qs, sb * qs, cos, sa, sb)):
        tab_ref[k] = t

    xl[0].wait()
    xbuf[0] = xst[0].astype(BF)
    pl.semaphore_wait(bar, 3)
    for u in (1, 2, 3):
        xsend(u).start()

    def wprep(u, i):
        @pl.when(u == 0)
        def _():
            wl[i].wait()
            wbf[i] = wst[i].astype(BF)
            if i == 2:
                xl[1].wait()
                xbuf[7] = xst[1].astype(BF)
                for k in (4, 5, 6):
                    xsend(k).start()

    def unit(u, carry):
        @pl.when(jnp.logical_and(u > 0, u < 7))
        def _():
            pltpu.make_async_copy(xbuf.at[u], xbuf.at[u], xr_sem.at[u]).wait()

        xb = xbuf[u]
        for w in range(3):
            wprep(u, w)
            for c in range(4):
                t = jnp.dot(xb, wbf[w, :, c * 256:(c + 1) * 256], preferred_element_type=F32)
                if w < 2:
                    cs, sa, sb = tab_ref[3 * w], tab_ref[3 * w + 1], tab_ref[3 * w + 2]
                    for hh in range(2):
                        th = t[:, hh * 128:(hh + 1) * 128]
                        r = th * cs + pltpu.roll(th, 127, 1) * sa + pltpu.roll(th, 1, 1) * sb
                        qkv[w, 2 * c + hh] = r.astype(BF)
                else:
                    for hh in range(2):
                        qkv[w, 2 * c + hh] = t[:, hh * 128:(hh + 1) * 128].astype(BF)
        for h in range(H):
            s = lax.dot_general(qkv[0, h], qkv[1, h], (((1,), (1,)), ((), ())),
                                preferred_element_type=F32)
            m = jnp.max(s, axis=1, keepdims=True)
            p = jnp.exp2(s - m)
            l = jnp.sum(p, axis=1, keepdims=True)
            o = jnp.dot(p.astype(BF), qkv[2, h], preferred_element_type=F32)
            ctx[:, h * 128:(h + 1) * 128] = (o / l).astype(BF)

        wprep(u, 3)

        @pl.when(u < 7)
        def _():
            for c in range(4):
                pbuf[u, :, c * 256:(c + 1) * 256] = jnp.dot(
                    ctx[...], wbf[3, :, c * 256:(c + 1) * 256], preferred_element_type=F32).astype(BF)

        @pl.when(jnp.logical_and(u > 0, u < 7))
        def _():
            off = jnp.where(u == 1, 3, jnp.where(u == 5, 3, jnp.where(jnp.logical_or(u == 2, u == 6), 1, 2)))
            psend(u, off).start()

        @pl.when(u == 5)
        def _():
            for k in (1, 2, 3):
                pltpu.make_async_copy(rbuf.at[k], rbuf.at[k], pr_sem.at[k]).wait()
            obuf[0] = (pbuf[0].astype(F32) + rbuf[1].astype(F32)) + (rbuf[2].astype(F32) + rbuf[3].astype(F32))
            pltpu.make_async_copy(obuf.at[0], out_hbm.at[0], osem.at[0]).start()

        return carry

    lax.fori_loop(0, NU, unit, 0)

    for k in (4, 5, 6):
        pltpu.make_async_copy(rbuf.at[k], rbuf.at[k], pr_sem.at[k]).wait()
    ocp = []
    for c in range(4):
        sl = slice(c * 256, (c + 1) * 256)
        t = jnp.dot(ctx[...], wbf[3, :, sl], preferred_element_type=F32)
        obuf[1, :, sl] = (t + rbuf[4, :, sl].astype(F32)) + (rbuf[5, :, sl].astype(F32) + rbuf[6, :, sl].astype(F32))
        cp = pltpu.make_async_copy(obuf.at[1, :, sl], out_hbm.at[1, :, sl], osem.at[1 + c])
        cp.start()
        ocp.append(cp)
    for u in range(1, 7):
        xsend(u).wait_send()
        psend(u, _OFF[u]).wait_send()
    pltpu.make_async_copy(obuf.at[0], out_hbm.at[0], osem.at[0]).wait()
    for cp in ocp:
        cp.wait()


def pallas_dist_rope_attn_htp_bs_b2_sq512_d1024_hq8_dh128_kernel(x, Wq, Wk, Wv, Wo):
    anyspec = pl.BlockSpec(memory_space=pl.ANY)
    return pl.pallas_call(
        _body,
        out_shape=jax.ShapeDtypeStruct((2, S, D), F32),
        in_specs=[anyspec] * 5,
        out_specs=anyspec,
        scratch_shapes=[
            pltpu.VMEM((6, S, DH), F32),
            pltpu.VMEM((2, S, D), F32),
            pltpu.VMEM((4, D, D), F32),
            pltpu.VMEM((4, D, D), BF),
            pltpu.VMEM((NU, S, D), BF),
            pltpu.VMEM((3, H, S, DH), BF),
            pltpu.VMEM((S, D), BF),
            pltpu.VMEM((NU - 1, S, D), BF),
            pltpu.VMEM((NU - 1, S, D), BF),
            pltpu.VMEM((2, S, D), F32),
            pltpu.SemaphoreType.DMA((6,)),
            pltpu.SemaphoreType.DMA((5,)),
            pltpu.SemaphoreType.DMA((NU,)),
            pltpu.SemaphoreType.DMA((NU,)),
            pltpu.SemaphoreType.DMA((NU,)),
            pltpu.SemaphoreType.DMA((NU,)),
        ],
        compiler_params=pltpu.CompilerParams(collective_id=0, vmem_limit_bytes=100 * 1024 * 1024),
    )(x, Wq, Wk, Wv, Wo)
```

```python
import jax
import jax.numpy as jnp
import numpy as np
from jax import lax
from jax.experimental import pallas as pl
from jax.experimental.pallas import tpu as pltpu

S, D, H, DH = 512, 1024, 8, 128
NU = 8
BF = jnp.bfloat16
F32 = jnp.float32


def _tables():
    inv = 1.0 / (10000.0 ** (np.arange(0, DH, 2) / DH))
    pos = np.arange(S)[:, None] * inv[None, :]
    cos = np.repeat(np.cos(pos), 2, axis=-1)
    sin = np.repeat(np.sin(pos), 2, axis=-1)
    even = (np.arange(DH) % 2 == 0)[None, :]
    sa = np.where(even, -sin, 0.0)
    sb = np.where(even, 0.0, sin)
    c = 0.08838834764831843 * 1.4426950408889634
    return np.stack([cos * c, sa * c, sb * c, cos, sa, sb]).astype(np.float32)


_TAB = _tables()

_OFF = (0, 3, 1, 2, 2, 3, 1, 0)
_BAT = (0, 0, 0, 0, 1, 1, 1, 1)


def _body(x_hbm, wq_hbm, wk_hbm, wv_hbm, wo_hbm, tab_hbm, out_hbm,
          tab_ref, xst, wst, wbf, xbuf, qkv, ctx, pbuf, rbuf, obuf,
          lsem, osem, xs_sem, xr_sem, ps_sem, pr_sem):
    me = lax.axis_index("i")

    def dev(off):
        return ((me + off) % 4,)

    bar = pltpu.get_barrier_semaphore()
    for off in (1, 2, 3):
        pl.semaphore_signal(bar, inc=1, device_id=dev(off), device_id_type=pl.DeviceIdType.MESH)

    xl = [pltpu.make_async_copy(x_hbm.at[b], xst.at[b], lsem.at[b]) for b in range(2)]
    wl = [pltpu.make_async_copy(w, wst.at[i], lsem.at[2 + i])
          for i, w in enumerate((wq_hbm, wk_hbm, wv_hbm, wo_hbm))]
    xl[0].start()
    wl[0].start()
    tl = pltpu.make_async_copy(tab_hbm, tab_ref, lsem.at[6])
    tl.start()
    wl[1].start()
    xl[1].start()
    wl[2].start()
    wl[3].start()

    def xsend(u):
        src = 0 if _BAT[u] == 0 else 7
        return pltpu.make_async_remote_copy(
            src_ref=xbuf.at[src], dst_ref=xbuf.at[u], send_sem=xs_sem.at[u], recv_sem=xr_sem.at[u],
            device_id=dev(4 - _OFF[u]), device_id_type=pl.DeviceIdType.MESH)

    def psend(u, off):
        return pltpu.make_async_remote_copy(
            src_ref=pbuf.at[u], dst_ref=rbuf.at[u], send_sem=ps_sem.at[u], recv_sem=pr_sem.at[u],
            device_id=dev(off), device_id_type=pl.DeviceIdType.MESH)

    xl[0].wait()
    xbuf[0] = xst[0].astype(BF)
    pl.semaphore_wait(bar, 3)
    for u in (1, 2, 3):
        xsend(u).start()

    def wprep(u, i):
        @pl.when(u == 0)
        def _():
            wl[i].wait()
            wbf[i] = wst[i].astype(BF)
            if i == 0:
                tl.wait()
            if i == 2:
                xl[1].wait()
                xbuf[7] = xst[1].astype(BF)
                for k in (4, 5, 6):
                    xsend(k).start()

    def unit(u, carry):
        @pl.when(jnp.logical_and(u > 0, u < 7))
        def _():
            pltpu.make_async_copy(xbuf.at[u], xbuf.at[u], xr_sem.at[u]).wait()

        xb = xbuf[u]
        for w in range(3):
            wprep(u, w)
            for c in range(4):
                t = jnp.dot(xb, wbf[w, :, c * 256:(c + 1) * 256], preferred_element_type=F32)
                if w < 2:
                    cs, sa, sb = tab_ref[3 * w], tab_ref[3 * w + 1], tab_ref[3 * w + 2]
                    for hh in range(2):
                        th = t[:, hh * 128:(hh + 1) * 128]
                        r = th * cs + pltpu.roll(th, 127, 1) * sa + pltpu.roll(th, 1, 1) * sb
                        qkv[w, 2 * c + hh] = r.astype(BF)
                else:
                    for hh in range(2):
                        qkv[w, 2 * c + hh] = t[:, hh * 128:(hh + 1) * 128].astype(BF)
        for h in range(H):
            s = lax.dot_general(qkv[0, h], qkv[1, h], (((1,), (1,)), ((), ())),
                                preferred_element_type=F32)
            m = jnp.max(s, axis=1, keepdims=True)
            p = jnp.exp2(s - m)
            l = jnp.sum(p, axis=1, keepdims=True)
            o = jnp.dot(p.astype(BF), qkv[2, h], preferred_element_type=F32)
            ctx[:, h * 128:(h + 1) * 128] = (o / l).astype(BF)

        wprep(u, 3)

        @pl.when(u < 7)
        def _():
            for c in range(4):
                pbuf[u, :, c * 256:(c + 1) * 256] = jnp.dot(
                    ctx[...], wbf[3, :, c * 256:(c + 1) * 256], preferred_element_type=F32).astype(BF)

        @pl.when(jnp.logical_and(u > 0, u < 7))
        def _():
            off = jnp.where(u == 1, 3, jnp.where(u == 5, 3, jnp.where(jnp.logical_or(u == 2, u == 6), 1, 2)))
            psend(u, off).start()

        @pl.when(u == 5)
        def _():
            for k in (1, 2, 3):
                pltpu.make_async_copy(rbuf.at[k], rbuf.at[k], pr_sem.at[k]).wait()
            obuf[0] = (pbuf[0].astype(F32) + rbuf[1].astype(F32)) + (rbuf[2].astype(F32) + rbuf[3].astype(F32))
            pltpu.make_async_copy(obuf.at[0], out_hbm.at[0], osem.at[0]).start()

        return carry

    lax.fori_loop(0, NU, unit, 0)

    for k in (4, 5, 6):
        pltpu.make_async_copy(rbuf.at[k], rbuf.at[k], pr_sem.at[k]).wait()
    ocp = []
    for c in range(4):
        sl = slice(c * 256, (c + 1) * 256)
        t = jnp.dot(ctx[...], wbf[3, :, sl], preferred_element_type=F32)
        obuf[1, :, sl] = (t + rbuf[4, :, sl].astype(F32)) + (rbuf[5, :, sl].astype(F32) + rbuf[6, :, sl].astype(F32))
        cp = pltpu.make_async_copy(obuf.at[1, :, sl], out_hbm.at[1, :, sl], osem.at[1 + c])
        cp.start()
        ocp.append(cp)
    for u in range(1, 7):
        xsend(u).wait_send()
        psend(u, _OFF[u]).wait_send()
    pltpu.make_async_copy(obuf.at[0], out_hbm.at[0], osem.at[0]).wait()
    for cp in ocp:
        cp.wait()


def pallas_dist_rope_attn_htp_bs_b2_sq512_d1024_hq8_dh128_kernel(x, Wq, Wk, Wv, Wo):
    anyspec = pl.BlockSpec(memory_space=pltpu.MemorySpace.HBM)
    return pl.pallas_call(
        _body,
        out_shape=jax.ShapeDtypeStruct((2, S, D), F32),
        in_specs=[anyspec] * 6,
        out_specs=anyspec,
        scratch_shapes=[
            pltpu.VMEM((6, S, DH), F32),
            pltpu.VMEM((2, S, D), F32),
            pltpu.VMEM((4, D, D), F32),
            pltpu.VMEM((4, D, D), BF),
            pltpu.VMEM((NU, S, D), BF),
            pltpu.VMEM((3, H, S, DH), BF),
            pltpu.VMEM((S, D), BF),
            pltpu.VMEM((NU - 1, S, D), BF),
            pltpu.VMEM((NU - 1, S, D), BF),
            pltpu.VMEM((2, S, D), F32),
            pltpu.SemaphoreType.DMA((7,)),
            pltpu.SemaphoreType.DMA((5,)),
            pltpu.SemaphoreType.DMA((NU,)),
            pltpu.SemaphoreType.DMA((NU,)),
            pltpu.SemaphoreType.DMA((NU,)),
            pltpu.SemaphoreType.DMA((NU,)),
        ],
        compiler_params=pltpu.CompilerParams(collective_id=0, vmem_limit_bytes=100 * 1024 * 1024),
    )(x, Wq, Wk, Wv, Wo, jnp.asarray(_TAB))
```

```python
import jax
import jax.numpy as jnp
import numpy as np
from jax import lax
from jax.experimental import pallas as pl
from jax.experimental.pallas import tpu as pltpu

S, D, H, DH = 512, 1024, 8, 128
NU = 8
BF = jnp.bfloat16
F32 = jnp.float32


def _tables():
    inv = 1.0 / (10000.0 ** (np.arange(0, DH, 2) / DH))
    pos = np.arange(S)[:, None] * inv[None, :]
    cos = np.repeat(np.cos(pos), 2, axis=-1)
    sin = np.repeat(np.sin(pos), 2, axis=-1)
    even = (np.arange(DH) % 2 == 0)[None, :]
    sa = np.where(even, -sin, 0.0)
    sb = np.where(even, 0.0, sin)
    c = 0.08838834764831843 * 1.4426950408889634
    return np.stack([cos * c, sa * c, sb * c, cos, sa, sb]).astype(np.float32)


_TAB = _tables()

_OFF = (0, 3, 1, 2, 2, 3, 1, 0)
_BAT = (0, 0, 0, 0, 1, 1, 1, 1)


def _body(x_hbm, wq_hbm, wk_hbm, wv_hbm, wo_hbm, tab_hbm, obuf,
          tab_ref, xst, wst, wbf, xbuf, qkv, ctx, pbuf, rbuf,
          lsem, xs_sem, xr_sem, ps_sem, pr_sem):
    me = lax.axis_index("i")

    def dev(off):
        return ((me + off) % 4,)

    bar = pltpu.get_barrier_semaphore()
    for off in (1, 2, 3):
        pl.semaphore_signal(bar, inc=1, device_id=dev(off), device_id_type=pl.DeviceIdType.MESH)

    xl = [pltpu.make_async_copy(x_hbm.at[b], xst.at[b], lsem.at[b]) for b in range(2)]
    wl = [pltpu.make_async_copy(w, wst.at[i], lsem.at[2 + i])
          for i, w in enumerate((wq_hbm, wk_hbm, wv_hbm, wo_hbm))]
    xl[0].start()
    wl[0].start()
    tl = pltpu.make_async_copy(tab_hbm, tab_ref, lsem.at[6])
    tl.start()
    wl[1].start()
    xl[1].start()
    wl[2].start()
    wl[3].start()

    def xsend(u):
        src = 0 if _BAT[u] == 0 else 7
        return pltpu.make_async_remote_copy(
            src_ref=xbuf.at[src], dst_ref=xbuf.at[u], send_sem=xs_sem.at[u], recv_sem=xr_sem.at[u],
            device_id=dev(4 - _OFF[u]), device_id_type=pl.DeviceIdType.MESH)

    def psend(u, off):
        return pltpu.make_async_remote_copy(
            src_ref=pbuf.at[u], dst_ref=rbuf.at[u], send_sem=ps_sem.at[u], recv_sem=pr_sem.at[u],
            device_id=dev(off), device_id_type=pl.DeviceIdType.MESH)

    xl[0].wait()
    xbuf[0] = xst[0].astype(BF)
    pl.semaphore_wait(bar, 3)
    for u in (1, 2, 3):
        xsend(u).start()

    def wprep(u, i):
        @pl.when(u == 0)
        def _():
            wl[i].wait()
            wbf[i] = wst[i].astype(BF)
            if i == 0:
                tl.wait()
            if i == 2:
                xl[1].wait()
                xbuf[7] = xst[1].astype(BF)
                for k in (4, 5, 6):
                    xsend(k).start()

    def unit(u, carry):
        @pl.when(jnp.logical_and(u > 0, u < 7))
        def _():
            pltpu.make_async_copy(xbuf.at[u], xbuf.at[u], xr_sem.at[u]).wait()

        xb = xbuf[u]
        for w in range(3):
            wprep(u, w)
            for c in range(4):
                t = jnp.dot(xb, wbf[w, :, c * 256:(c + 1) * 256], preferred_element_type=F32)
                if w < 2:
                    cs, sa, sb = tab_ref[3 * w], tab_ref[3 * w + 1], tab_ref[3 * w + 2]
                    for hh in range(2):
                        th = t[:, hh * 128:(hh + 1) * 128]
                        r = th * cs + pltpu.roll(th, 127, 1) * sa + pltpu.roll(th, 1, 1) * sb
                        qkv[w, 2 * c + hh] = r.astype(BF)
                else:
                    for hh in range(2):
                        qkv[w, 2 * c + hh] = t[:, hh * 128:(hh + 1) * 128].astype(BF)
        for h in range(H):
            s = lax.dot_general(qkv[0, h], qkv[1, h], (((1,), (1,)), ((), ())),
                                preferred_element_type=F32)
            m = jnp.max(s, axis=1, keepdims=True)
            p = jnp.exp2(s - m)
            l = jnp.sum(p, axis=1, keepdims=True)
            o = jnp.dot(p.astype(BF), qkv[2, h], preferred_element_type=F32)
            ctx[:, h * 128:(h + 1) * 128] = (o / l).astype(BF)

        wprep(u, 3)

        @pl.when(u < 7)
        def _():
            for c in range(4):
                pbuf[u, :, c * 256:(c + 1) * 256] = jnp.dot(
                    ctx[...], wbf[3, :, c * 256:(c + 1) * 256], preferred_element_type=F32).astype(BF)

        @pl.when(jnp.logical_and(u > 0, u < 7))
        def _():
            off = jnp.where(u == 1, 3, jnp.where(u == 5, 3, jnp.where(jnp.logical_or(u == 2, u == 6), 1, 2)))
            psend(u, off).start()

        @pl.when(u == 5)
        def _():
            for k in (1, 2, 3):
                pltpu.make_async_copy(rbuf.at[k], rbuf.at[k], pr_sem.at[k]).wait()
            obuf[0] = (pbuf[0].astype(F32) + rbuf[1].astype(F32)) + (rbuf[2].astype(F32) + rbuf[3].astype(F32))

        return carry

    lax.fori_loop(0, NU, unit, 0)

    for k in (4, 5, 6):
        pltpu.make_async_copy(rbuf.at[k], rbuf.at[k], pr_sem.at[k]).wait()
    for c in range(4):
        sl = slice(c * 256, (c + 1) * 256)
        t = jnp.dot(ctx[...], wbf[3, :, sl], preferred_element_type=F32)
        obuf[1, :, sl] = (t + rbuf[4, :, sl].astype(F32)) + (rbuf[5, :, sl].astype(F32) + rbuf[6, :, sl].astype(F32))
    for u in range(1, 7):
        xsend(u).wait_send()
        psend(u, _OFF[u]).wait_send()


def pallas_dist_rope_attn_htp_bs_b2_sq512_d1024_hq8_dh128_kernel(x, Wq, Wk, Wv, Wo):
    anyspec = pl.BlockSpec(memory_space=pltpu.MemorySpace.HBM)
    return pl.pallas_call(
        _body,
        out_shape=pltpu.VMEM((2, S, D), F32),
        in_specs=[anyspec] * 6,
        out_specs=pl.BlockSpec(memory_space=pltpu.VMEM),
        scratch_shapes=[
            pltpu.VMEM((6, S, DH), F32),
            pltpu.VMEM((2, S, D), F32),
            pltpu.VMEM((4, D, D), F32),
            pltpu.VMEM((4, D, D), BF),
            pltpu.VMEM((NU, S, D), BF),
            pltpu.VMEM((3, H, S, DH), BF),
            pltpu.VMEM((S, D), BF),
            pltpu.VMEM((NU - 1, S, D), BF),
            pltpu.VMEM((NU - 1, S, D), BF),
            pltpu.SemaphoreType.DMA((7,)),
            pltpu.SemaphoreType.DMA((NU,)),
            pltpu.SemaphoreType.DMA((NU,)),
            pltpu.SemaphoreType.DMA((NU,)),
            pltpu.SemaphoreType.DMA((NU,)),
        ],
        compiler_params=pltpu.CompilerParams(collective_id=0, vmem_limit_bytes=100 * 1024 * 1024),
    )(x, Wq, Wk, Wv, Wo, jnp.asarray(_TAB))
```

```python
import jax
import jax.numpy as jnp
import numpy as np
from jax import lax
from jax.experimental import pallas as pl
from jax.experimental.pallas import tpu as pltpu

S, D, H, DH = 512, 1024, 8, 128
NU = 8
CW = 256
NC = D // CW
HPC = CW // DH
BF = jnp.bfloat16
F32 = jnp.float32


def _tables():
    inv = 1.0 / (10000.0 ** (np.arange(0, DH, 2) / DH))
    pos = np.arange(S)[:, None] * inv[None, :]
    cos = np.repeat(np.cos(pos), 2, axis=-1)
    sin = np.repeat(np.sin(pos), 2, axis=-1)
    even = (np.arange(DH) % 2 == 0)[None, :]
    sa = np.where(even, -sin, 0.0)
    sb = np.where(even, 0.0, sin)
    c = 0.08838834764831843 * 1.4426950408889634
    return np.stack([cos * c, sa * c, sb * c, cos, sa, sb]).astype(np.float32)


_TAB = _tables()

_OFF = (0, 3, 1, 2, 2, 3, 1, 0)
_BAT = (0, 0, 0, 0, 1, 1, 1, 1)


def _body(x_hbm, wq_hbm, wk_hbm, wv_hbm, wo_hbm, tab_hbm, obuf,
          tab_ref, xst, wst, wbf, xbuf, pbuf, rbuf,
          lsem, xs_sem, xr_sem, ps_sem, pr_sem):
    me = lax.axis_index("i")

    def dev(off):
        return ((me + off) % 4,)

    bar = pltpu.get_barrier_semaphore()
    for off in (1, 2, 3):
        pl.semaphore_signal(bar, inc=1, device_id=dev(off), device_id_type=pl.DeviceIdType.MESH)

    xl = [pltpu.make_async_copy(x_hbm.at[b], xst.at[b], lsem.at[b]) for b in range(2)]
    tl = pltpu.make_async_copy(tab_hbm, tab_ref, lsem.at[2])
    wol = pltpu.make_async_copy(wo_hbm, wst.at[3], lsem.at[3])
    wl = {(w, c): pltpu.make_async_copy(r.at[:, c * CW:(c + 1) * CW], wst.at[w, :, c * CW:(c + 1) * CW],
                                        lsem.at[4 + 3 * c + w])
          for c in range(NC) for w, r in enumerate((wq_hbm, wk_hbm, wv_hbm))}
    xl[0].start()
    for c in range(NC):
        for w in range(3):
            wl[w, c].start()
            if c == 0 and w == 0:
                tl.start()
    wol.start()
    xl[1].start()

    def xsend(u):
        src = 0 if _BAT[u] == 0 else 7
        return pltpu.make_async_remote_copy(
            src_ref=xbuf.at[src], dst_ref=xbuf.at[u], send_sem=xs_sem.at[u], recv_sem=xr_sem.at[u],
            device_id=dev(4 - _OFF[u]), device_id_type=pl.DeviceIdType.MESH)

    def psend(u, off):
        return pltpu.make_async_remote_copy(
            src_ref=pbuf.at[u], dst_ref=rbuf.at[u], send_sem=ps_sem.at[u], recv_sem=pr_sem.at[u],
            device_id=dev(off), device_id_type=pl.DeviceIdType.MESH)

    xl[0].wait()
    xbuf[0] = xst[0].astype(BF)
    pl.semaphore_wait(bar, 3)
    for u in (1, 2, 3):
        xsend(u).start()

    def proj(xb, c, first):
        sl = slice(c * CW, (c + 1) * CW)
        res = []
        for w in range(3):
            if first:
                wl[w, c].wait()
                wbf[w, :, sl] = wst[w, :, sl].astype(BF)
                if c == 0 and w == 0:
                    tl.wait()
            t = jnp.dot(xb, wbf[w, :, sl], preferred_element_type=F32)
            hs = []
            for hh in range(HPC):
                th = t[:, hh * DH:(hh + 1) * DH]
                if w < 2:
                    cs, sa, sb = tab_ref[3 * w], tab_ref[3 * w + 1], tab_ref[3 * w + 2]
                    th = th * cs + pltpu.roll(th, DH - 1, 1) * sa + pltpu.roll(th, 1, 1) * sb
                hs.append(th.astype(BF))
            res.append(hs)
        return res

    def attn(qkv):
        outs = []
        for hh in range(HPC):
            s = lax.dot_general(qkv[0][hh], qkv[1][hh], (((1,), (1,)), ((), ())),
                                preferred_element_type=F32)
            m = jnp.max(s, axis=1, keepdims=True)
            p = jnp.exp2(s - m)
            l = jnp.sum(p, axis=1, keepdims=True)
            o = jnp.dot(p.astype(BF), qkv[2][hh], preferred_element_type=F32)
            outs.append((o / l).astype(BF))
        return outs

    def heads(xb, first):
        cx = []
        nxt = proj(xb, 0, first)
        for c in range(NC - 1):
            cur, nxt = nxt, proj(xb, c + 1, first)
            cx += attn(cur)
        if first:
            wol.wait()
            wbf[3] = wst[3].astype(BF)
        ks = (NC - 1) * CW
        acc = jnp.dot(jnp.concatenate(cx, axis=1), wbf[3, :ks, :], preferred_element_type=F32)
        last = jnp.concatenate(attn(nxt), axis=1)
        return acc, last, ks

    def full_unit(u, first):
        acc, last, ks = heads(xbuf[u], first)
        pbuf[u] = (acc + jnp.dot(last, wbf[3, ks:, :], preferred_element_type=F32)).astype(BF)

    full_unit(0, True)

    def unit(u, carry):
        pltpu.make_async_copy(xbuf.at[u], xbuf.at[u], xr_sem.at[u]).wait()

        @pl.when(u == 1)
        def _():
            xl[1].wait()
            xbuf[7] = xst[1].astype(BF)
            for k in (4, 5, 6):
                xsend(k).start()

        @pl.when(u == 5)
        def _():
            for k in (1, 2, 3):
                pltpu.make_async_copy(rbuf.at[k], rbuf.at[k], pr_sem.at[k]).wait()
            obuf[0] = (pbuf[0].astype(F32) + rbuf[1].astype(F32)) + (rbuf[2].astype(F32) + rbuf[3].astype(F32))

        full_unit(u, False)
        off = jnp.where(jnp.logical_or(u == 1, u == 5), 3, jnp.where(jnp.logical_or(u == 2, u == 6), 1, 2))
        psend(u, off).start()
        return carry

    lax.fori_loop(1, NU - 1, unit, 0)

    acc, last, ks = heads(xbuf[7], False)
    for k in (4, 5, 6):
        pltpu.make_async_copy(rbuf.at[k], rbuf.at[k], pr_sem.at[k]).wait()
    obuf[1] = ((acc + jnp.dot(last, wbf[3, ks:, :], preferred_element_type=F32) + rbuf[4].astype(F32))
               + (rbuf[5].astype(F32) + rbuf[6].astype(F32)))
    for u in range(1, 7):
        xsend(u).wait_send()
        psend(u, _OFF[u]).wait_send()


def pallas_dist_rope_attn_htp_bs_b2_sq512_d1024_hq8_dh128_kernel(x, Wq, Wk, Wv, Wo):
    anyspec = pl.BlockSpec(memory_space=pltpu.MemorySpace.HBM)
    return pl.pallas_call(
        _body,
        out_shape=pltpu.VMEM((2, S, D), F32),
        in_specs=[anyspec] * 6,
        out_specs=pl.BlockSpec(memory_space=pltpu.VMEM),
        scratch_shapes=[
            pltpu.VMEM((6, S, DH), F32),
            pltpu.VMEM((2, S, D), F32),
            pltpu.VMEM((4, D, D), F32),
            pltpu.VMEM((4, D, D), BF),
            pltpu.VMEM((NU, S, D), BF),
            pltpu.VMEM((NU - 1, S, D), BF),
            pltpu.VMEM((NU - 1, S, D), BF),
            pltpu.SemaphoreType.DMA((4 + 3 * NC,)),
            pltpu.SemaphoreType.DMA((NU,)),
            pltpu.SemaphoreType.DMA((NU,)),
            pltpu.SemaphoreType.DMA((NU,)),
            pltpu.SemaphoreType.DMA((NU,)),
        ],
        compiler_params=pltpu.CompilerParams(collective_id=0, vmem_limit_bytes=100 * 1024 * 1024),
    )(x, Wq, Wk, Wv, Wo, jnp.asarray(_TAB))
```

```python
import jax
import jax.numpy as jnp
import numpy as np
from jax import lax
from jax.experimental import pallas as pl
from jax.experimental.pallas import tpu as pltpu

S, D, H, DH = 512, 1024, 8, 128
NU = 8
BF = jnp.bfloat16
F32 = jnp.float32


def _tables():
    inv = 1.0 / (10000.0 ** (np.arange(0, DH, 2) / DH))
    pos = np.arange(S)[:, None] * inv[None, :]
    cos = np.repeat(np.cos(pos), 2, axis=-1)
    sin = np.repeat(np.sin(pos), 2, axis=-1)
    even = (np.arange(DH) % 2 == 0)[None, :]
    sa = np.where(even, -sin, 0.0)
    sb = np.where(even, 0.0, sin)
    c = 0.08838834764831843 * 1.4426950408889634
    return np.stack([cos * c, sa * c, sb * c, cos, sa, sb]).astype(np.float32)


_TAB = _tables()

_OFF = (0, 3, 1, 2, 2, 3, 1, 0)
_BAT = (0, 0, 0, 0, 1, 1, 1, 1)


def _body(x_hbm, wq_hbm, wk_hbm, wv_hbm, wo_hbm, tab_hbm, obuf,
          tab_ref, xst, wst, wbf, xbuf, qkv, ctx, pbuf, rbuf,
          lsem, xs_sem, xr_sem, ps_sem, pr_sem):
    me = lax.axis_index("i")

    def dev(off):
        return ((me + off) % 4,)

    bar = pltpu.get_barrier_semaphore()
    for off in (1, 2, 3):
        pl.semaphore_signal(bar, inc=1, device_id=dev(off), device_id_type=pl.DeviceIdType.MESH)

    xl = [pltpu.make_async_copy(x_hbm.at[b], xst.at[b], lsem.at[b]) for b in range(2)]
    wl = [pltpu.make_async_copy(w, wst.at[i], lsem.at[2 + i])
          for i, w in enumerate((wq_hbm, wk_hbm, wv_hbm, wo_hbm))]
    xl[0].start()
    wl[0].start()
    tl = pltpu.make_async_copy(tab_hbm, tab_ref, lsem.at[6])
    tl.start()
    wl[1].start()
    wl[2].start()
    wl[3].start()
    xl[1].start()

    def xsend(u):
        src = 0 if _BAT[u] == 0 else 7
        return pltpu.make_async_remote_copy(
            src_ref=xbuf.at[src], dst_ref=xbuf.at[u], send_sem=xs_sem.at[u], recv_sem=xr_sem.at[u],
            device_id=dev(4 - _OFF[u]), device_id_type=pl.DeviceIdType.MESH)

    def psend(u, off):
        return pltpu.make_async_remote_copy(
            src_ref=pbuf.at[u], dst_ref=rbuf.at[u], send_sem=ps_sem.at[u], recv_sem=pr_sem.at[u],
            device_id=dev(off), device_id_type=pl.DeviceIdType.MESH)

    xl[0].wait()
    xbuf[0] = xst[0].astype(BF)
    pl.semaphore_wait(bar, 3)
    for u in (1, 2):
        xsend(u).start()

    def wprep(u, i):
        @pl.when(u == 0)
        def _():
            wl[i].wait()
            wbf[i] = wst[i].astype(BF)
            if i == 0:
                tl.wait()

    def unit(u, carry):
        @pl.when(jnp.logical_and(u > 0, u < 7))
        def _():
            pltpu.make_async_copy(xbuf.at[u], xbuf.at[u], xr_sem.at[u]).wait()

        @pl.when(u == 1)
        def _():
            xsend(3).start()
            xl[1].wait()
            xbuf[7] = xst[1].astype(BF)

        @pl.when(u == 2)
        def _():
            xsend(4).start()

        @pl.when(u == 3)
        def _():
            xsend(5).start()
            xsend(6).start()

        xb = xbuf[u]
        for w in range(3):
            wprep(u, w)
            for c in range(4):
                t = jnp.dot(xb, wbf[w, :, c * 256:(c + 1) * 256], preferred_element_type=F32)
                if w < 2:
                    cs, sa, sb = tab_ref[3 * w], tab_ref[3 * w + 1], tab_ref[3 * w + 2]
                    for hh in range(2):
                        th = t[:, hh * 128:(hh + 1) * 128]
                        r = th * cs + pltpu.roll(th, 127, 1) * sa + pltpu.roll(th, 1, 1) * sb
                        qkv[w, 2 * c + hh] = r.astype(BF)
                else:
                    for hh in range(2):
                        qkv[w, 2 * c + hh] = t[:, hh * 128:(hh + 1) * 128].astype(BF)
        for h in range(H):
            s = lax.dot_general(qkv[0, h], qkv[1, h], (((1,), (1,)), ((), ())),
                                preferred_element_type=F32)
            m = jnp.max(s, axis=1, keepdims=True)
            p = jnp.exp2(s - m)
            l = jnp.sum(p, axis=1, keepdims=True)
            o = jnp.dot(p.astype(BF), qkv[2, h], preferred_element_type=F32)
            ctx[:, h * 128:(h + 1) * 128] = (o / l).astype(BF)

        wprep(u, 3)

        @pl.when(u < 7)
        def _():
            for c in range(4):
                pbuf[u, :, c * 256:(c + 1) * 256] = jnp.dot(
                    ctx[...], wbf[3, :, c * 256:(c + 1) * 256], preferred_element_type=F32).astype(BF)

        @pl.when(jnp.logical_and(u > 0, u < 7))
        def _():
            off = jnp.where(u == 1, 3, jnp.where(u == 5, 3, jnp.where(jnp.logical_or(u == 2, u == 6), 1, 2)))
            psend(u, off).start()

        @pl.when(u == 6)
        def _():
            for k in (1, 2, 3):
                pltpu.make_async_copy(rbuf.at[k], rbuf.at[k], pr_sem.at[k]).wait()
            obuf[0] = (pbuf[0].astype(F32) + rbuf[1].astype(F32)) + (rbuf[2].astype(F32) + rbuf[3].astype(F32))

        return carry

    lax.fori_loop(0, NU, unit, 0)

    for k in (4, 5, 6):
        pltpu.make_async_copy(rbuf.at[k], rbuf.at[k], pr_sem.at[k]).wait()
    for c in range(4):
        sl = slice(c * 256, (c + 1) * 256)
        t = jnp.dot(ctx[...], wbf[3, :, sl], preferred_element_type=F32)
        obuf[1, :, sl] = (t + rbuf[4, :, sl].astype(F32)) + (rbuf[5, :, sl].astype(F32) + rbuf[6, :, sl].astype(F32))
    for u in range(1, 7):
        xsend(u).wait_send()
        psend(u, _OFF[u]).wait_send()


def pallas_dist_rope_attn_htp_bs_b2_sq512_d1024_hq8_dh128_kernel(x, Wq, Wk, Wv, Wo):
    anyspec = pl.BlockSpec(memory_space=pl.ANY)
    return pl.pallas_call(
        _body,
        out_shape=pltpu.VMEM((2, S, D), F32),
        in_specs=[anyspec] * 6,
        out_specs=pl.BlockSpec(memory_space=pltpu.VMEM),
        scratch_shapes=[
            pltpu.VMEM((6, S, DH), F32),
            pltpu.VMEM((2, S, D), F32),
            pltpu.VMEM((4, D, D), F32),
            pltpu.VMEM((4, D, D), BF),
            pltpu.VMEM((NU, S, D), BF),
            pltpu.VMEM((3, H, S, DH), BF),
            pltpu.VMEM((S, D), BF),
            pltpu.VMEM((NU - 1, S, D), BF),
            pltpu.VMEM((NU - 1, S, D), BF),
            pltpu.SemaphoreType.DMA((7,)),
            pltpu.SemaphoreType.DMA((NU,)),
            pltpu.SemaphoreType.DMA((NU,)),
            pltpu.SemaphoreType.DMA((NU,)),
            pltpu.SemaphoreType.DMA((NU,)),
        ],
        compiler_params=pltpu.CompilerParams(collective_id=0, vmem_limit_bytes=100 * 1024 * 1024),
    )(x, Wq, Wk, Wv, Wo, jnp.asarray(_TAB))
```

```python
import jax
import jax.numpy as jnp
import numpy as np
from jax import lax
from jax.experimental import pallas as pl
from jax.experimental.pallas import tpu as pltpu

S, D, H, DH = 512, 1024, 8, 128
NU = 8
BF = jnp.bfloat16
F32 = jnp.float32


def _tables():
    inv = 1.0 / (10000.0 ** (np.arange(0, DH, 2) / DH))
    pos = np.arange(S)[:, None] * inv[None, :]
    cos = np.repeat(np.cos(pos), 2, axis=-1)
    sin = np.repeat(np.sin(pos), 2, axis=-1)
    even = (np.arange(DH) % 2 == 0)[None, :]
    sa = np.where(even, -sin, 0.0)
    sb = np.where(even, 0.0, sin)
    c = 0.08838834764831843 * 1.4426950408889634
    return np.stack([cos * c, sa * c, sb * c, cos, sa, sb]).astype(np.float32)


_TAB = _tables()

_OFF = (0, 3, 1, 2, 2, 3, 1, 0)
_BAT = (0, 0, 0, 0, 1, 1, 1, 1)


def _body(x_hbm, wq_hbm, wk_hbm, wv_hbm, wo_hbm, tab_hbm, obuf,
          tab_ref, xst, wst, wbf, xbuf, qkv, ctx, pbuf, rbuf,
          lsem, xs_sem, xr_sem, ps_sem, pr_sem):
    me = lax.axis_index("i")

    def dev(off):
        return ((me + off) % 4,)

    bar = pltpu.get_barrier_semaphore()
    for off in (1, 2, 3):
        pl.semaphore_signal(bar, inc=1, device_id=dev(off), device_id_type=pl.DeviceIdType.MESH)

    xl = [pltpu.make_async_copy(x_hbm.at[b], xst.at[b], lsem.at[b]) for b in range(2)]
    wl = [pltpu.make_async_copy(w, wst.at[i], lsem.at[2 + i])
          for i, w in enumerate((wq_hbm, wk_hbm, wv_hbm, wo_hbm))]
    xl[0].start()
    wl[0].start()
    tl = pltpu.make_async_copy(tab_hbm, tab_ref, lsem.at[6])
    tl.start()
    wl[1].start()
    wl[2].start()
    wl[3].start()
    xl[1].start()

    def xsend(u):
        src = 0 if _BAT[u] == 0 else 7
        return pltpu.make_async_remote_copy(
            src_ref=xbuf.at[src], dst_ref=xbuf.at[u], send_sem=xs_sem.at[u], recv_sem=xr_sem.at[u],
            device_id=dev(4 - _OFF[u]), device_id_type=pl.DeviceIdType.MESH)

    def psend(u, off):
        return pltpu.make_async_remote_copy(
            src_ref=pbuf.at[u], dst_ref=rbuf.at[u], send_sem=ps_sem.at[u], recv_sem=pr_sem.at[u],
            device_id=dev(off), device_id_type=pl.DeviceIdType.MESH)

    xl[0].wait()
    xbuf[0] = xst[0].astype(BF)
    pl.semaphore_wait(bar, 3)
    for u in (1, 2, 3):
        xsend(u).start()

    def wprep(u, i):
        @pl.when(u == 0)
        def _():
            wl[i].wait()
            wbf[i] = wst[i].astype(BF)
            if i == 0:
                tl.wait()

    def unit(u, carry):
        @pl.when(jnp.logical_and(u > 0, u < 7))
        def _():
            pltpu.make_async_copy(xbuf.at[u], xbuf.at[u], xr_sem.at[u]).wait()

        @pl.when(u == 1)
        def _():
            xl[1].wait()
            xbuf[7] = xst[1].astype(BF)

        @pl.when(u == 1)
        def _():
            xsend(4).start()

        @pl.when(u == 1)
        def _():
            xsend(5).start()
            xsend(6).start()

        xb = xbuf[u]
        for w in range(3):
            wprep(u, w)
            for c in range(4):
                t = jnp.dot(xb, wbf[w, :, c * 256:(c + 1) * 256], preferred_element_type=F32)
                if w < 2:
                    cs, sa, sb = tab_ref[3 * w], tab_ref[3 * w + 1], tab_ref[3 * w + 2]
                    for hh in range(2):
                        th = t[:, hh * 128:(hh + 1) * 128]
                        r = th * cs + pltpu.roll(th, 127, 1) * sa + pltpu.roll(th, 1, 1) * sb
                        qkv[w, 2 * c + hh] = r.astype(BF)
                else:
                    for hh in range(2):
                        qkv[w, 2 * c + hh] = t[:, hh * 128:(hh + 1) * 128].astype(BF)
        for h in range(H):
            s = lax.dot_general(qkv[0, h], qkv[1, h], (((1,), (1,)), ((), ())),
                                preferred_element_type=F32)
            m = jnp.max(s, axis=1, keepdims=True)
            p = jnp.exp2(s - m)
            l = jnp.sum(p, axis=1, keepdims=True)
            o = jnp.dot(p.astype(BF), qkv[2, h], preferred_element_type=F32)
            ctx[:, h * 128:(h + 1) * 128] = (o / l).astype(BF)

        wprep(u, 3)

        @pl.when(u < 7)
        def _():
            for c in range(4):
                pbuf[u, :, c * 256:(c + 1) * 256] = jnp.dot(
                    ctx[...], wbf[3, :, c * 256:(c + 1) * 256], preferred_element_type=F32).astype(BF)

        @pl.when(jnp.logical_and(u > 0, u < 7))
        def _():
            off = jnp.where(u == 1, 3, jnp.where(u == 5, 3, jnp.where(jnp.logical_or(u == 2, u == 6), 1, 2)))
            psend(u, off).start()

        @pl.when(u == 6)
        def _():
            for k in (1, 2, 3):
                pltpu.make_async_copy(rbuf.at[k], rbuf.at[k], pr_sem.at[k]).wait()
            obuf[0] = (pbuf[0].astype(F32) + rbuf[1].astype(F32)) + (rbuf[2].astype(F32) + rbuf[3].astype(F32))

        return carry

    lax.fori_loop(0, NU, unit, 0)

    for k in (4, 5, 6):
        pltpu.make_async_copy(rbuf.at[k], rbuf.at[k], pr_sem.at[k]).wait()
    for c in range(4):
        sl = slice(c * 256, (c + 1) * 256)
        t = jnp.dot(ctx[...], wbf[3, :, sl], preferred_element_type=F32)
        obuf[1, :, sl] = (t + rbuf[4, :, sl].astype(F32)) + (rbuf[5, :, sl].astype(F32) + rbuf[6, :, sl].astype(F32))
    for u in range(1, 7):
        xsend(u).wait_send()
        psend(u, _OFF[u]).wait_send()


def pallas_dist_rope_attn_htp_bs_b2_sq512_d1024_hq8_dh128_kernel(x, Wq, Wk, Wv, Wo):
    anyspec = pl.BlockSpec(memory_space=pl.ANY)
    return pl.pallas_call(
        _body,
        out_shape=pltpu.VMEM((2, S, D), F32),
        in_specs=[anyspec] * 6,
        out_specs=pl.BlockSpec(memory_space=pltpu.VMEM),
        scratch_shapes=[
            pltpu.VMEM((6, S, DH), F32),
            pltpu.VMEM((2, S, D), F32),
            pltpu.VMEM((4, D, D), F32),
            pltpu.VMEM((4, D, D), BF),
            pltpu.VMEM((NU, S, D), BF),
            pltpu.VMEM((3, H, S, DH), BF),
            pltpu.VMEM((S, D), BF),
            pltpu.VMEM((NU - 1, S, D), BF),
            pltpu.VMEM((NU - 1, S, D), BF),
            pltpu.SemaphoreType.DMA((7,)),
            pltpu.SemaphoreType.DMA((NU,)),
            pltpu.SemaphoreType.DMA((NU,)),
            pltpu.SemaphoreType.DMA((NU,)),
            pltpu.SemaphoreType.DMA((NU,)),
        ],
        compiler_params=pltpu.CompilerParams(collective_id=0, vmem_limit_bytes=100 * 1024 * 1024),
    )(x, Wq, Wk, Wv, Wo, jnp.asarray(_TAB))
```

```python
import jax
import jax.numpy as jnp
import numpy as np
from jax import lax
from jax.experimental import pallas as pl
from jax.experimental.pallas import tpu as pltpu

S, D, H, DH = 512, 1024, 8, 128
NU = 8
CW = 256
NC = D // CW
KH = 6
HPC = CW // DH
BF = jnp.bfloat16
F32 = jnp.float32


def _tables():
    inv = 1.0 / (10000.0 ** (np.arange(0, DH, 2) / DH))
    pos = np.arange(S)[:, None] * inv[None, :]
    cos = np.repeat(np.cos(pos), 2, axis=-1)
    sin = np.repeat(np.sin(pos), 2, axis=-1)
    even = (np.arange(DH) % 2 == 0)[None, :]
    return np.where(even, cos, sin).astype(np.float32)


_TAB = _tables()

_OFF = (0, 3, 1, 2, 2, 3, 1, 0)
_BAT = (0, 0, 0, 0, 1, 1, 1, 1)


def _body(x_hbm, wq_hbm, wk_hbm, wv_hbm, wo_hbm, tab_hbm, obuf,
          tab_ref, xst, wst, wbf, xbuf, qkv, pbuf, rbuf,
          lsem, xs_sem, xr_sem, ps_sem, pr_sem):
    me = lax.axis_index("i")

    def dev(off):
        return ((me + off) % 4,)

    bar = pltpu.get_barrier_semaphore()
    for off in (1, 2, 3):
        pl.semaphore_signal(bar, inc=1, device_id=dev(off), device_id_type=pl.DeviceIdType.MESH)

    xl = [pltpu.make_async_copy(x_hbm.at[b], xst.at[b], lsem.at[b]) for b in range(2)]
    tl = pltpu.make_async_copy(tab_hbm, tab_ref.at[0], lsem.at[2])
    wl = {(w, c): pltpu.make_async_copy(r.at[:, c * CW:(c + 1) * CW], wst.at[w, :, c * CW:(c + 1) * CW],
                                        lsem.at[3 + 4 * c + w])
          for c in range(NC) for w, r in enumerate((wq_hbm, wk_hbm, wv_hbm))}
    for c in range(NC):
        wl[3, c] = pltpu.make_async_copy(wo_hbm.at[c * CW:(c + 1) * CW], wst.at[3, c * CW:(c + 1) * CW],
                                         lsem.at[3 + 4 * c + 3])
    tl.start()
    xl[0].start()
    order = [(w, 0) for w in range(3)]
    for c in range(1, NC):
        order += [(w, c) for w in range(3)] + [(3, c - 1)]
    order += [(3, NC - 1)]
    for k in order:
        wl[k].start()
    xl[1].start()

    def xsend(u):
        if u == 3:
            return pltpu.make_async_remote_copy(
                src_ref=xbuf.at[1], dst_ref=xbuf.at[3], send_sem=xs_sem.at[3], recv_sem=xr_sem.at[3],
                device_id=dev(1), device_id_type=pl.DeviceIdType.MESH)
        if u == 4:
            return pltpu.make_async_remote_copy(
                src_ref=xbuf.at[6], dst_ref=xbuf.at[4], send_sem=xs_sem.at[4], recv_sem=xr_sem.at[4],
                device_id=dev(3), device_id_type=pl.DeviceIdType.MESH)
        src = 0 if _BAT[u] == 0 else 7
        return pltpu.make_async_remote_copy(
            src_ref=xbuf.at[src], dst_ref=xbuf.at[u], send_sem=xs_sem.at[u], recv_sem=xr_sem.at[u],
            device_id=dev(4 - _OFF[u]), device_id_type=pl.DeviceIdType.MESH)

    def psend(u, off):
        return pltpu.make_async_remote_copy(
            src_ref=pbuf.at[u], dst_ref=rbuf.at[u], send_sem=ps_sem.at[u], recv_sem=pr_sem.at[u],
            device_id=dev(off), device_id_type=pl.DeviceIdType.MESH)

    tl.wait()
    tp = tab_ref[0]
    even = (lax.broadcasted_iota(jnp.int32, (S, DH), 1) & 1) == 0
    cos = jnp.where(even, tp, pltpu.roll(tp, 1, 1))
    sa = jnp.where(even, -pltpu.roll(tp, DH - 1, 1), 0.0)
    sb = jnp.where(even, 0.0, tp)
    qs = 0.08838834764831843 * 1.4426950408889634
    for k, t in enumerate((cos * qs, sa * qs, sb * qs, cos, sa, sb)):
        tab_ref[k] = t

    xl[0].wait()
    xbuf[0] = xst[0].astype(BF)
    pl.semaphore_wait(bar, 3)
    for u in (1, 2):
        xsend(u).start()

    def proj(xb, w, c, first):
        sl = slice(c * CW, (c + 1) * CW)
        if first:
            wl[w, c].wait()
            wv = wst[w, :, sl].astype(BF)
            wbf[w, :, sl] = wv
        else:
            wv = wbf[w, :, sl]
        t = jnp.dot(xb, wv, preferred_element_type=F32)
        for hh in range(HPC):
            th = t[:, hh * DH:(hh + 1) * DH]
            if w < 2:
                cs, sa, sb = tab_ref[3 * w], tab_ref[3 * w + 1], tab_ref[3 * w + 2]
                th = th * cs + pltpu.roll(th, DH - 1, 1) * sa + pltpu.roll(th, 1, 1) * sb
            qkv[w, c * HPC + hh] = th.astype(BF)

    def attn(h):
        s = lax.dot_general(qkv[0, h], qkv[1, h], (((1,), (1,)), ((), ())),
                            preferred_element_type=F32)
        m = jnp.max(s, axis=1, keepdims=True)
        p = jnp.exp2(s - m)
        l = jnp.sum(p, axis=1, keepdims=True)
        o = jnp.dot(p.astype(BF), qkv[2, h], preferred_element_type=F32)
        return (o * pl.reciprocal(l, approx=True)).astype(BF)

    def heads(xb):
        for w in range(3):
            for c in range(NC):
                proj(xb, w, c, False)
        cx = [attn(h) for h in range(KH)]
        ks = KH * DH
        acc = jnp.dot(jnp.concatenate(cx, axis=1), wbf[3, :ks, :], preferred_element_type=F32)
        last = jnp.concatenate([attn(h) for h in range(KH, H)], axis=1)
        return acc, last, ks

    def full_unit(u):
        acc, last, ks = heads(xbuf[u])
        pbuf[u] = (acc + jnp.dot(last, wbf[3, ks:, :], preferred_element_type=F32)).astype(BF)

        @pl.when(u == 6)
        def _():
            pltpu.make_async_copy(rbuf.at[4], rbuf.at[4], pr_sem.at[4]).wait()
            pbuf[6] = (pbuf[6].astype(F32) + rbuf[4].astype(F32)).astype(BF)

    xb0 = xbuf[0]
    for w in range(3):
        proj(xb0, w, 0, True)
    for c in range(NC):
        if c + 1 < NC:
            for w in range(3):
                proj(xb0, w, c + 1, True)
        cg = jnp.concatenate([attn(h) for h in range(c * HPC, (c + 1) * HPC)], axis=1)
        wl[3, c].wait()
        wv = wst[3, c * CW:(c + 1) * CW, :].astype(BF)
        wbf[3, c * CW:(c + 1) * CW, :] = wv
        t = jnp.dot(cg, wv, preferred_element_type=F32)
        obuf[0] = t if c == 0 else obuf[0] + t

    def unit(u, carry):
        @pl.when(u != 6)
        def _():
            pltpu.make_async_copy(xbuf.at[u], xbuf.at[u], xr_sem.at[u]).wait()

        @pl.when(u == 1)
        def _():
            xsend(3).start()
            xl[1].wait()
            xbuf[7] = xst[1].astype(BF)
            xsend(6).start()
            xsend(5).start()

        @pl.when(u == 3)
        def _():
            pltpu.make_async_copy(xbuf.at[6], xbuf.at[6], xr_sem.at[6]).wait()
            xsend(4).start()

        full_unit(u)
        off = jnp.where(jnp.logical_or(u == 1, u == 5), 3, jnp.where(u == 3, 2, 1))
        psend(u, off).start()
        return carry

    lax.fori_loop(1, NU - 1, unit, 0)

    for k in (1, 2, 3):
        pltpu.make_async_copy(rbuf.at[k], rbuf.at[k], pr_sem.at[k]).wait()
    obuf[0] = (obuf[0] + rbuf[1].astype(F32)) + (rbuf[2].astype(F32) + rbuf[3].astype(F32))
    acc, last, ks = heads(xbuf[7])
    obuf[1] = acc + jnp.dot(last, wbf[3, ks:, :], preferred_element_type=F32)
    for k in (5, 6):
        pltpu.make_async_copy(rbuf.at[k], rbuf.at[k], pr_sem.at[k]).wait()
    obuf[1] = obuf[1] + (rbuf[5].astype(F32) + rbuf[6].astype(F32))
    for u in range(1, 7):
        xsend(u).wait_send()
        psend(u, 1 if u == 4 else _OFF[u]).wait_send()


def pallas_dist_rope_attn_htp_bs_b2_sq512_d1024_hq8_dh128_kernel(x, Wq, Wk, Wv, Wo):
    anyspec = pl.BlockSpec(memory_space=pltpu.MemorySpace.HBM)
    return pl.pallas_call(
        _body,
        out_shape=pltpu.VMEM((2, S, D), F32),
        in_specs=[anyspec] * 6,
        out_specs=pl.BlockSpec(memory_space=pltpu.VMEM),
        scratch_shapes=[
            pltpu.VMEM((6, S, DH), F32),
            pltpu.VMEM((2, S, D), F32),
            pltpu.VMEM((4, D, D), F32),
            pltpu.VMEM((4, D, D), BF),
            pltpu.VMEM((NU, S, D), BF),
            pltpu.VMEM((3, H, S, DH), BF),
            pltpu.VMEM((NU - 1, S, D), BF),
            pltpu.VMEM((NU - 1, S, D), BF),
            pltpu.SemaphoreType.DMA((3 + 4 * NC,)),
            pltpu.SemaphoreType.DMA((NU,)),
            pltpu.SemaphoreType.DMA((NU,)),
            pltpu.SemaphoreType.DMA((NU,)),
            pltpu.SemaphoreType.DMA((NU,)),
        ],
        compiler_params=pltpu.CompilerParams(collective_id=0, vmem_limit_bytes=100 * 1024 * 1024),
    )(x, Wq, Wk, Wv, Wo, jnp.asarray(_TAB))
```
